```python
import numpy as np

kernel_name = "dist_moe_cap_ep_outshard_n2048_d512_e8_h1024"

def setup_inputs():
    x = np.random.randn(2048, 512).astype(np.float32)
    router_W = np.random.randn(512, 32).astype(np.float32) * 0.1
    scores64 = x.astype(np.float64) @ router_W.astype(np.float64)
    route_idx = np.argsort(-scores64, axis=-1)[:, :1].astype(np.int32)
    expert_W = np.random.randn(32, 512, 1024).astype(np.float32) * 0.02
    return {"x": x, "router_W": router_W, "route_idx": route_idx, "expert_W": expert_W}

def reference(x, router_W, route_idx, expert_W):
    counts = np.zeros(32, dtype=np.int64)
    out = np.zeros((2048, 1024), dtype=np.float32)
    for i in range(2048):
        e = int(route_idx[i, 0])
        if counts[e] < 51:
            out[i] = x[i] @ expert_W[e]
            counts[e] += 1
    return out
```

```python
import os
import contextlib
import jax
import jax.numpy as jnp
from jax import lax
from jax.experimental import pallas as pl
from jax.experimental.pallas import tpu as pltpu

N_TOK = 2048
D = 512
H = 1024
N_EXP = 32
N_DEV = 4
E_LOC = N_EXP // N_DEV
CAP = 51
SLOTS = 64
PAIRS = SLOTS // 2
TOK_LOC = N_TOK // N_DEV
KC = 4
KB = D // KC
NBLK = N_TOK // 128
GPAIRS = (CAP + 1) // 2
PROF = os.environ.get("KPROF", "0") == "1"


def scope(name):
    return jax.named_scope(name) if PROF else contextlib.nullcontext()


def _body(idx_ref, x_hbm, w_hbm, out_ref,
          wbuf, xg, sb, rb, meta_v, meta_s,
          wsem, xsem, ssem, rsem, msem):
    me = lax.axis_index("i")

    def w_copy(i):
        e, kc = divmod(i, KC)
        return pltpu.make_async_copy(
            w_hbm.at[e, pl.ds(kc * KB, KB), :], wbuf.at[e, pl.ds(kc * KB, KB), :], wsem.at[i])

    for i in range(E_LOC * KC):
        w_copy(i).start(priority=1)

    barrier = pltpu.get_barrier_semaphore()
    for d in range(1, N_DEV):
        pl.semaphore_signal(barrier, inc=1, device_id=((me + d) % N_DEV,),
                            device_id_type=pl.DeviceIdType.MESH)

    with scope("meta"):
        idx = idx_ref[...]
        e_iota = lax.broadcasted_iota(jnp.int32, (NBLK, N_EXP, 128), 1)
        oh = (idx[:, None, :] == e_iota)
        oh_f = jnp.where(oh, 1.0, 0.0).astype(jnp.float32)
        oh2 = oh_f.reshape(NBLK * N_EXP, 128).astype(jnp.bfloat16)
        r_i = lax.broadcasted_iota(jnp.int32, (128, 128), 0)
        c_i = lax.broadcasted_iota(jnp.int32, (128, 128), 1)
        upper = jnp.where(r_i < c_i, 1.0, 0.0).astype(jnp.bfloat16)
        ones = jnp.ones((128, 128), jnp.bfloat16)
        cw = jnp.dot(oh2, upper, preferred_element_type=jnp.float32).reshape(NBLK, N_EXP, 128)
        tot = jnp.dot(oh2, ones, preferred_element_type=jnp.float32).reshape(NBLK, N_EXP, 128)
        carry = jnp.zeros((N_EXP, 128), jnp.float32)
        lane = lax.broadcasted_iota(jnp.int32, (N_EXP, 128), 1)
        bnd = jnp.zeros((N_EXP, 128), jnp.float32)
        slot_iota = lax.broadcasted_iota(jnp.int32, (SLOTS, 128), 0)
        lane_f = lane.astype(jnp.float32)
        a_parts, b_parts = [], []
        for b in range(NBLK):
            if b % (NBLK // N_DEV) == 0:
                bnd = jnp.where(lane == SLOTS + b // (NBLK // N_DEV),
                                jnp.minimum(carry, float(CAP)), bnd)
            cum = cw[b] + carry
            pos = jnp.sum(oh_f[b] * cum, axis=0, keepdims=True)
            pos_i = pos.astype(jnp.int32)
            bt = jnp.where((slot_iota == pos_i) & (slot_iota < CAP), 1.0, 0.0).astype(jnp.bfloat16)
            a_b = jnp.concatenate([oh_f[b] * float(b), oh_f[b] * lane_f], axis=0).astype(jnp.bfloat16)
            a_parts.append(a_b)
            b_parts.append(bt)
            carry = carry + tot[b]
        bnd = jnp.where(lane == SLOTS + N_DEV, jnp.minimum(carry, float(CAP)), bnd)
        a_all = jnp.concatenate(a_parts, axis=1)
        b_all = jnp.concatenate(b_parts, axis=1)
        tk = lax.dot_general(a_all, b_all, (((1,), (1,)), ((), ())),
                             preferred_element_type=jnp.float32)
        tok = tk[:N_EXP] * 128.0 + tk[N_EXP:]
        tok_pad = jnp.concatenate([tok, jnp.zeros((N_EXP, 128 - SLOTS), jnp.float32)], axis=1)
        m0 = jnp.where(lane < SLOTS, tok_pad, bnd).astype(jnp.int32)
        m1 = ((m0 & (TOK_LOC - 1)) >> 3) * 64 + (m0 & 7)
        meta_v[pl.ds(0, N_EXP), :] = m0
        meta_v[pl.ds(N_EXP, N_EXP), :] = m1
        mcp = pltpu.make_async_copy(meta_v, meta_s, msem)
        mcp.start()

    with scope("zero"):
        xg[...] = jnp.zeros(xg.shape, xg.dtype)
        out_ref[...] = jnp.zeros(out_ref.shape, out_ref.dtype)
        mcp.wait()

    with scope("gissue"):
        for e in range(E_LOC):
            ge = me * E_LOC + e

            def issue(p, carry_, e=e, ge=ge):
                t0 = meta_s[ge, 2 * p]
                t1 = meta_s[ge, 2 * p + 1]
                pltpu.make_async_copy(x_hbm.at[pl.ds(t0, 1)], xg.at[pl.ds(e * SLOTS + p, 1)],
                                      xsem.at[e]).start()
                pltpu.make_async_copy(x_hbm.at[pl.ds(t1, 1)],
                                      xg.at[pl.ds(e * SLOTS + PAIRS + p, 1)], xsem.at[e]).start()
                return carry_
            lax.fori_loop(0, GPAIRS, issue, 0, unroll=2)

    with scope("barrier"):
        pl.semaphore_wait(barrier, N_DEV - 1)

    def send_copy(e, d):
        k = (me + d) % N_DEV
        ge = me * E_LOC + e
        s0 = meta_s[ge, SLOTS + k]
        s1 = meta_s[ge, SLOTS + k + 1]
        ps = s0 >> 1
        npair = ((s1 + 1) >> 1) - ps
        src = sb.at[pl.ds(pl.multiple_of((e * PAIRS + ps) * 8, 8), npair * 8)]
        dst = rb.at[pl.ds(pl.multiple_of((ge * PAIRS + ps) * 8, 8), npair * 8)]
        if d == 0:
            cp = pltpu.make_async_copy(src, dst, rsem.at[me * E_LOC + e])
        else:
            cp = pltpu.make_async_remote_copy(
                src_ref=src, dst_ref=dst, send_sem=ssem.at[e * N_DEV + d],
                recv_sem=rsem.at[me * E_LOC + e], device_id=(k,),
                device_id_type=pl.DeviceIdType.MESH)
        return cp, s1 > s0

    def receive(e):
        for s in range(N_DEV):
            ge = s * E_LOC + e
            s0 = meta_s[ge, SLOTS + me]
            s1 = meta_s[ge, SLOTS + me + 1]

            @pl.when(s1 > s0)
            def _(ge=ge, s0=s0, s1=s1):
                ps = s0 >> 1
                npair = ((s1 + 1) >> 1) - ps
                dst = rb.at[pl.ds(pl.multiple_of((ge * PAIRS + ps) * 8, 8), npair * 8)]
                pltpu.make_async_copy(dst, dst, rsem.at[ge]).wait()

                def place(c, carry_):
                    off = meta_s[N_EXP + ge, c]
                    u = rb[pl.ds(pl.multiple_of((ge * PAIRS + (c >> 1)) * 8, 8), 8), :]
                    sh = ((c & 1) << 4).astype(jnp.uint32)
                    v = lax.bitcast_convert_type(
                        (u << sh) & jnp.uint32(0xFFFF0000), jnp.float32)
                    out_ref[pl.ds(off, 8, stride=8), :] = v
                    return carry_
                lax.fori_loop(s0, s1, place, 0)

    for e in range(E_LOC):
        with scope(f"xwait{e}"):
            rows = xg.at[pl.ds(0, 2 * GPAIRS // 8 * 8)]
            pltpu.make_async_copy(rows, rows, xsem.at[e]).wait()
            for _ in range(2 * GPAIRS % 8):
                row1 = xg.at[pl.ds(0, 1)]
                pltpu.make_async_copy(row1, row1, xsem.at[e]).wait()

        with scope(f"mm{e}"):
            xb = xg[pl.ds(e * SLOTS, SLOTS), :].astype(jnp.bfloat16)
            acc = None
            for kc in range(KC):
                i = e * KC + kc
                w_copy(i).wait()
                wb = wbuf[e, pl.ds(kc * KB, KB), :].astype(jnp.bfloat16)
                part = jnp.dot(xb[:, kc * KB:(kc + 1) * KB], wb, preferred_element_type=jnp.float32)
                acc = part if acc is None else acc + part
            hi = lax.bitcast_convert_type(
                acc[:PAIRS].astype(jnp.bfloat16).astype(jnp.float32), jnp.uint32)
            lo = lax.bitcast_convert_type(
                acc[PAIRS:].astype(jnp.bfloat16).astype(jnp.float32), jnp.uint32)
            packed = hi | (lo >> jnp.uint32(16))
            for g in range(PAIRS // 8):
                for j in range(H // 128):
                    sb[pl.ds(e * PAIRS * 8 + g * 64 + j, 8, stride=8), :] = (
                        packed[8 * g:8 * g + 8, 128 * j:128 * (j + 1)])
        with scope(f"send{e}"):
            for d in range(N_DEV):
                cp, nonempty = send_copy(e, d)
                pl.when(nonempty)(cp.start)
        if e > 0:
            with scope(f"recv{e - 1}"):
                receive(e - 1)
    with scope("recv7"):
        receive(E_LOC - 1)

    with scope("drain"):
        for e in range(E_LOC):
            for d in range(1, N_DEV):
                cp, nonempty = send_copy(e, d)
                pl.when(nonempty)(cp.wait_send)


def pallas_dist_moe_cap_ep_outshard_n2048_d512_e8_h1024_kernel(x, router_W, route_idx, expert_W):
    del router_W
    idx2d = route_idx.astype(jnp.int32).reshape(NBLK, 128)
    out = pl.pallas_call(
        _body,
        out_shape=jax.ShapeDtypeStruct((TOK_LOC * 8, 128), jnp.float32),
        in_specs=[pl.BlockSpec(memory_space=pltpu.VMEM),
                  pl.BlockSpec(memory_space=pl.ANY),
                  pl.BlockSpec(memory_space=pl.ANY)],
        out_specs=pl.BlockSpec(memory_space=pltpu.VMEM),
        scratch_shapes=[
            pltpu.VMEM((E_LOC, D, H), jnp.float32),
            pltpu.VMEM((E_LOC * SLOTS, D), jnp.float32),
            pltpu.VMEM((E_LOC * PAIRS * 8, 128), jnp.uint32),
            pltpu.VMEM((N_EXP * PAIRS * 8, 128), jnp.uint32),
            pltpu.VMEM((2 * N_EXP, 128), jnp.int32),
            pltpu.SMEM((2 * N_EXP, 128), jnp.int32),
            pltpu.SemaphoreType.DMA((E_LOC * KC,)),
            pltpu.SemaphoreType.DMA((E_LOC,)),
            pltpu.SemaphoreType.DMA((E_LOC * N_DEV,)),
            pltpu.SemaphoreType.DMA((N_EXP,)),
            pltpu.SemaphoreType.DMA,
        ],
        compiler_params=pltpu.CompilerParams(
            collective_id=0, vmem_limit_bytes=64 * 1024 * 1024, disable_bounds_checks=True, disable_semaphore_checks=True),
    )(idx2d, x, expert_W)
    out = out.reshape(TOK_LOC // 8, H // 128, 8, 128).transpose(0, 2, 1, 3)
    return out.reshape(TOK_LOC, H)
```

```python
import jax
import jax.numpy as jnp
from jax import lax
from jax.experimental import pallas as pl
from jax.experimental.pallas import tpu as pltpu

N_TOK = 2048
D = 512
H = 1024
N_EXP = 32
N_DEV = 4
E_LOC = N_EXP // N_DEV
CAP = 51
SLOTS = 64
PAIRS = SLOTS // 2
TOK_LOC = N_TOK // N_DEV
NBLK = N_TOK // 128
GPAIRS = (CAP + 1) // 2
KCS = (1, 1, 1, 1, 1, 2, 2, 4)
W_CHUNKS = [(e, kc * (D // n), D // n) for e, n in enumerate(KCS) for kc in range(n)]


def _body(idx_ref, x_hbm, w_hbm, out_ref,
          wbuf, xg, sb, rb, meta_v, meta_s,
          wsem, xsem, ssem, rsem, msem):
    me = lax.axis_index("i")

    def w_copy(i):
        e, k0, kb = W_CHUNKS[i]
        return pltpu.make_async_copy(
            w_hbm.at[e, pl.ds(k0, kb), :], wbuf.at[e, pl.ds(k0, kb), :], wsem.at[i])

    for i in range(len(W_CHUNKS)):
        w_copy(i).start(priority=1)

    barrier = pltpu.get_barrier_semaphore()
    for d in range(1, N_DEV):
        pl.semaphore_signal(barrier, inc=1, device_id=((me + d) % N_DEV,),
                            device_id_type=pl.DeviceIdType.MESH)

    idx = idx_ref[...]
    e_iota = lax.broadcasted_iota(jnp.int32, (NBLK, N_EXP, 128), 1)
    oh_f = jnp.where(idx[:, None, :] == e_iota, 1.0, 0.0).astype(jnp.float32)
    oh2 = oh_f.reshape(NBLK * N_EXP, 128).astype(jnp.bfloat16)
    r_i = lax.broadcasted_iota(jnp.int32, (128, 128), 0)
    c_i = lax.broadcasted_iota(jnp.int32, (128, 128), 1)
    upper = jnp.where(r_i < c_i, 1.0, 0.0).astype(jnp.bfloat16)
    ones = jnp.ones((128, 128), jnp.bfloat16)
    cw = jnp.dot(oh2, upper, preferred_element_type=jnp.float32).reshape(NBLK, N_EXP, 128)
    tot = jnp.dot(oh2, ones, preferred_element_type=jnp.float32).reshape(NBLK, N_EXP, 128)
    carry = jnp.zeros((N_EXP, 128), jnp.float32)
    lane = lax.broadcasted_iota(jnp.int32, (N_EXP, 128), 1)
    bnd = jnp.zeros((N_EXP, 128), jnp.float32)
    slot_iota = lax.broadcasted_iota(jnp.int32, (SLOTS, 128), 0)
    lane_f = lane.astype(jnp.float32)
    a_parts, b_parts = [], []
    for b in range(NBLK):
        if b % (NBLK // N_DEV) == 0:
            bnd = jnp.where(lane == SLOTS + b // (NBLK // N_DEV),
                            jnp.minimum(carry, float(CAP)), bnd)
        cum = cw[b] + carry
        pos = jnp.sum(oh_f[b] * cum, axis=0, keepdims=True)
        pos_i = pos.astype(jnp.int32)
        bt = jnp.where((slot_iota == pos_i) & (slot_iota < CAP), 1.0, 0.0).astype(jnp.bfloat16)
        a_b = jnp.concatenate([oh_f[b] * float(b), oh_f[b] * lane_f],
                              axis=0).astype(jnp.bfloat16)
        a_parts.append(a_b)
        b_parts.append(bt)
        carry = carry + tot[b]
    bnd = jnp.where(lane == SLOTS + N_DEV, jnp.minimum(carry, float(CAP)), bnd)
    a_all = jnp.concatenate(a_parts, axis=1)
    b_all = jnp.concatenate(b_parts, axis=1)
    tk = lax.dot_general(a_all, b_all, (((1,), (1,)), ((), ())),
                         preferred_element_type=jnp.float32)
    tok = tk[:N_EXP] * 128.0 + tk[N_EXP:]
    tok_pad = jnp.concatenate([tok, jnp.zeros((N_EXP, 128 - SLOTS), jnp.float32)], axis=1)
    m0 = jnp.where(lane < SLOTS, tok_pad, bnd).astype(jnp.int32)
    m1 = ((m0 & (TOK_LOC - 1)) >> 3) * 64 + (m0 & 7)
    meta_v[pl.ds(0, N_EXP), :] = m0
    meta_v[pl.ds(N_EXP, N_EXP), :] = m1
    mcp = pltpu.make_async_copy(meta_v, meta_s, msem)
    mcp.start()

    xg[...] = jnp.zeros(xg.shape, xg.dtype)
    out_ref[...] = jnp.zeros(out_ref.shape, out_ref.dtype)
    mcp.wait()

    for e in range(E_LOC):
        ge = me * E_LOC + e

        def issue(p, carry_, e=e, ge=ge):
            t0 = meta_s[ge, 2 * p]
            t1 = meta_s[ge, 2 * p + 1]
            pltpu.make_async_copy(x_hbm.at[pl.ds(t0, 1)], xg.at[pl.ds(e * SLOTS + p, 1)],
                                  xsem.at[e]).start()
            pltpu.make_async_copy(x_hbm.at[pl.ds(t1, 1)],
                                  xg.at[pl.ds(e * SLOTS + PAIRS + p, 1)], xsem.at[e]).start()
            return carry_
        lax.fori_loop(0, GPAIRS, issue, 0, unroll=2)

    pl.semaphore_wait(barrier, N_DEV - 1)

    def send_copy(e, d):
        k = (me + d) % N_DEV
        ge = me * E_LOC + e
        s0 = meta_s[ge, SLOTS + k]
        s1 = meta_s[ge, SLOTS + k + 1]
        ps = s0 >> 1
        npair = ((s1 + 1) >> 1) - ps
        src = sb.at[pl.ds(pl.multiple_of((e * PAIRS + ps) * 8, 8), npair * 8)]
        dst = rb.at[pl.ds(pl.multiple_of((ge * PAIRS + ps) * 8, 8), npair * 8)]
        if d == 0:
            cp = pltpu.make_async_copy(src, dst, rsem.at[ge])
        else:
            cp = pltpu.make_async_remote_copy(
                src_ref=src, dst_ref=dst, send_sem=ssem.at[e * N_DEV + d],
                recv_sem=rsem.at[ge], device_id=(k,),
                device_id_type=pl.DeviceIdType.MESH)
        return cp, s1 > s0

    def receive(e):
        for s in range(N_DEV):
            ge = s * E_LOC + e
            s0 = meta_s[ge, SLOTS + me]
            s1 = meta_s[ge, SLOTS + me + 1]

            @pl.when(s1 > s0)
            def _(ge=ge, s0=s0, s1=s1):
                ps = s0 >> 1
                npair = ((s1 + 1) >> 1) - ps
                dst = rb.at[pl.ds(pl.multiple_of((ge * PAIRS + ps) * 8, 8), npair * 8)]
                pltpu.make_async_copy(dst, dst, rsem.at[ge]).wait()

                def place(c, carry_):
                    off = meta_s[N_EXP + ge, c]
                    u = rb[pl.ds(pl.multiple_of((ge * PAIRS + (c >> 1)) * 8, 8), 8), :]
                    sh = ((c & 1) << 4).astype(jnp.uint32)
                    v = lax.bitcast_convert_type(
                        (u << sh) & jnp.uint32(0xFFFF0000), jnp.float32)
                    out_ref[pl.ds(off, 8, stride=8), :] = v
                    return carry_
                lax.fori_loop(s0, s1, place, 0)

    def drain(e):
        for d in range(1, N_DEV):
            cp, nonempty = send_copy(e, d)
            pl.when(nonempty)(cp.wait_send)

    for e in range(E_LOC):
        rows = xg.at[pl.ds(0, 2 * GPAIRS // 8 * 8)]
        pltpu.make_async_copy(rows, rows, xsem.at[e]).wait()
        for _ in range(2 * GPAIRS % 8):
            row1 = xg.at[pl.ds(0, 1)]
            pltpu.make_async_copy(row1, row1, xsem.at[e]).wait()

        xb = xg[pl.ds(e * SLOTS, SLOTS), :].astype(jnp.bfloat16)
        acc = None
        for i, (ce, k0, kb) in enumerate(W_CHUNKS):
            if ce != e:
                continue
            w_copy(i).wait()
            wb = wbuf[e, pl.ds(k0, kb), :].astype(jnp.bfloat16)
            part = jnp.dot(xb[:, k0:k0 + kb], wb, preferred_element_type=jnp.float32)
            acc = part if acc is None else acc + part
        hi = lax.bitcast_convert_type(
            acc[:PAIRS].astype(jnp.bfloat16).astype(jnp.float32), jnp.uint32)
        lo = lax.bitcast_convert_type(
            acc[PAIRS:].astype(jnp.bfloat16).astype(jnp.float32), jnp.uint32)
        packed = hi | (lo >> jnp.uint32(16))
        for g in range(PAIRS // 8):
            for j in range(H // 128):
                sb[pl.ds(e * PAIRS * 8 + g * 64 + j, 8, stride=8), :] = (
                    packed[8 * g:8 * g + 8, 128 * j:128 * (j + 1)])
        for d in (2, 1, 3, 0):
            cp, nonempty = send_copy(e, d)
            pl.when(nonempty)(cp.start)
        if e > 0:
            receive(e - 1)
            drain(e - 1)
    receive(E_LOC - 1)
    drain(E_LOC - 1)


def pallas_dist_moe_cap_ep_outshard_n2048_d512_e8_h1024_kernel(x, router_W, route_idx, expert_W):
    del router_W
    idx2d = route_idx.astype(jnp.int32).reshape(NBLK, 128)
    out = pl.pallas_call(
        _body,
        out_shape=jax.ShapeDtypeStruct((TOK_LOC * 8, 128), jnp.float32),
        in_specs=[pl.BlockSpec(memory_space=pltpu.VMEM),
                  pl.BlockSpec(memory_space=pl.ANY),
                  pl.BlockSpec(memory_space=pl.ANY)],
        out_specs=pl.BlockSpec(memory_space=pltpu.VMEM),
        scratch_shapes=[
            pltpu.VMEM((E_LOC, D, H), jnp.float32),
            pltpu.VMEM((E_LOC * SLOTS, D), jnp.float32),
            pltpu.VMEM((E_LOC * PAIRS * 8, 128), jnp.uint32),
            pltpu.VMEM((N_EXP * PAIRS * 8, 128), jnp.uint32),
            pltpu.VMEM((2 * N_EXP, 128), jnp.int32),
            pltpu.SMEM((2 * N_EXP, 128), jnp.int32),
            pltpu.SemaphoreType.DMA((len(W_CHUNKS),)),
            pltpu.SemaphoreType.DMA((E_LOC,)),
            pltpu.SemaphoreType.DMA((E_LOC * N_DEV,)),
            pltpu.SemaphoreType.DMA((N_EXP,)),
            pltpu.SemaphoreType.DMA,
        ],
        compiler_params=pltpu.CompilerParams(
            collective_id=0, vmem_limit_bytes=64 * 1024 * 1024,
            disable_bounds_checks=True, disable_semaphore_checks=True),
    )(idx2d, x, expert_W)
    out = out.reshape(TOK_LOC // 8, H // 128, 8, 128).transpose(0, 2, 1, 3)
    return out.reshape(TOK_LOC, H)
```

```python
import jax
import jax.numpy as jnp
from jax import lax
from jax.experimental import pallas as pl
from jax.experimental.pallas import tpu as pltpu

N_TOK = 2048
D = 512
H = 1024
N_EXP = 32
N_DEV = 4
E_LOC = N_EXP // N_DEV
CAP = 51
SLOTS = 64
PAIRS = SLOTS // 2
TOK_LOC = N_TOK // N_DEV
NBLK = N_TOK // 128
GPAIRS = (CAP + 1) // 2
KCS = (1, 1, 1, 1, 1, 2, 2, 4)
W_CHUNKS = [(e, kc * (D // n), D // n) for e, n in enumerate(KCS) for kc in range(n)]


def _body(idx_ref, x_hbm, w_hbm, out_ref,
          wbuf, xg, sb, rb, meta_v, meta_s,
          wsem, xsem, ssem, rsem, msem):
    me = lax.axis_index("i")

    def w_copy(i):
        e, k0, kb = W_CHUNKS[i]
        return pltpu.make_async_copy(
            w_hbm.at[e, pl.ds(k0, kb), :], wbuf.at[e, pl.ds(k0, kb), :], wsem.at[i])

    for i in range(len(W_CHUNKS)):
        w_copy(i).start(priority=1)

    barrier = pltpu.get_barrier_semaphore()
    for d in range(1, N_DEV):
        pl.semaphore_signal(barrier, inc=1, device_id=((me + d) % N_DEV,),
                            device_id_type=pl.DeviceIdType.MESH)

    idx = idx_ref[...]
    e_iota = lax.broadcasted_iota(jnp.int32, (NBLK, N_EXP, 128), 1)
    oh_f = jnp.where(idx[:, None, :] == e_iota, 1.0, 0.0).astype(jnp.float32)
    oh2 = oh_f.reshape(NBLK * N_EXP, 128).astype(jnp.bfloat16)
    r_i = lax.broadcasted_iota(jnp.int32, (128, 128), 0)
    c_i = lax.broadcasted_iota(jnp.int32, (128, 128), 1)
    upper = jnp.where(r_i < c_i, 1.0, 0.0).astype(jnp.bfloat16)
    ones = jnp.ones((128, 128), jnp.bfloat16)
    cw = jnp.dot(oh2, upper, preferred_element_type=jnp.float32).reshape(NBLK, N_EXP, 128)
    tot = jnp.dot(oh2, ones, preferred_element_type=jnp.float32).reshape(NBLK, N_EXP, 128)
    carry = jnp.zeros((N_EXP, 128), jnp.float32)
    lane = lax.broadcasted_iota(jnp.int32, (N_EXP, 128), 1)
    bnd = jnp.zeros((N_EXP, 128), jnp.float32)
    slot_iota = lax.broadcasted_iota(jnp.int32, (SLOTS, 128), 0)
    lane_f = lane.astype(jnp.float32)
    a_parts, b_parts = [], []
    for b in range(NBLK):
        if b % (NBLK // N_DEV) == 0:
            bnd = jnp.where(lane == SLOTS + b // (NBLK // N_DEV),
                            jnp.minimum(carry, float(CAP)), bnd)
        cum = cw[b] + carry
        pos = jnp.sum(oh_f[b] * cum, axis=0, keepdims=True)
        pos_i = pos.astype(jnp.int32)
        bt = jnp.where((slot_iota == pos_i) & (slot_iota < CAP), 1.0, 0.0).astype(jnp.bfloat16)
        a_b = jnp.concatenate([oh_f[b] * float(b), oh_f[b] * lane_f],
                              axis=0).astype(jnp.bfloat16)
        a_parts.append(a_b)
        b_parts.append(bt)
        carry = carry + tot[b]
    bnd = jnp.where(lane == SLOTS + N_DEV, jnp.minimum(carry, float(CAP)), bnd)
    a_all = jnp.concatenate(a_parts, axis=1)
    b_all = jnp.concatenate(b_parts, axis=1)
    tk = lax.dot_general(a_all, b_all, (((1,), (1,)), ((), ())),
                         preferred_element_type=jnp.float32)
    tok = tk[:N_EXP] * 128.0 + tk[N_EXP:]
    tok_pad = jnp.concatenate([tok, jnp.zeros((N_EXP, 128 - SLOTS), jnp.float32)], axis=1)
    m0 = jnp.where(lane < SLOTS, tok_pad, bnd).astype(jnp.int32)
    m1 = m0 & (TOK_LOC - 1)
    meta_v[pl.ds(0, N_EXP), :] = m0
    meta_v[pl.ds(N_EXP, N_EXP), :] = m1
    mcp = pltpu.make_async_copy(meta_v, meta_s, msem)
    mcp.start()

    xg[...] = jnp.zeros(xg.shape, xg.dtype)
    out_ref[...] = jnp.zeros(out_ref.shape, out_ref.dtype)
    mcp.wait()

    for e in range(E_LOC):
        ge = me * E_LOC + e

        def issue(p, carry_, e=e, ge=ge):
            t0 = meta_s[ge, 2 * p]
            t1 = meta_s[ge, 2 * p + 1]
            pltpu.make_async_copy(x_hbm.at[pl.ds(t0, 1)], xg.at[pl.ds(e * SLOTS + p, 1)],
                                  xsem.at[e]).start()
            pltpu.make_async_copy(x_hbm.at[pl.ds(t1, 1)],
                                  xg.at[pl.ds(e * SLOTS + PAIRS + p, 1)], xsem.at[e]).start()
            return carry_
        lax.fori_loop(0, GPAIRS, issue, 0, unroll=2)

    pl.semaphore_wait(barrier, N_DEV - 1)

    def send_copy(e, d):
        k = (me + d) % N_DEV
        ge = me * E_LOC + e
        s0 = meta_s[ge, SLOTS + k]
        s1 = meta_s[ge, SLOTS + k + 1]
        ps = s0 >> 1
        npair = ((s1 + 1) >> 1) - ps
        src = sb.at[pl.ds(e * PAIRS + ps, npair)]
        dst = rb.at[pl.ds(ge * PAIRS + ps, npair)]
        if d == 0:
            cp = pltpu.make_async_copy(src, dst, rsem.at[ge])
        else:
            cp = pltpu.make_async_remote_copy(
                src_ref=src, dst_ref=dst, send_sem=ssem.at[e * N_DEV + d],
                recv_sem=rsem.at[ge], device_id=(k,),
                device_id_type=pl.DeviceIdType.MESH)
        return cp, s1 > s0

    def receive(e):
        for s in range(N_DEV):
            ge = s * E_LOC + e
            s0 = meta_s[ge, SLOTS + me]
            s1 = meta_s[ge, SLOTS + me + 1]

            @pl.when(s1 > s0)
            def _(ge=ge, s0=s0, s1=s1):
                ps = s0 >> 1
                npair = ((s1 + 1) >> 1) - ps
                dst = rb.at[pl.ds(ge * PAIRS + ps, npair)]
                pltpu.make_async_copy(dst, dst, rsem.at[ge]).wait()

                def place(c, carry_):
                    row = meta_s[N_EXP + ge, c]
                    u = rb[ge * PAIRS + (c >> 1)]
                    sh = ((c & 1) << 4).astype(jnp.uint32)
                    v = lax.bitcast_convert_type(
                        (u << sh) & jnp.uint32(0xFFFF0000), jnp.float32)
                    out_ref[row >> 3, :, row & 7, :] = v
                    return carry_
                lax.fori_loop(s0, s1, place, 0)

    def drain(e):
        for d in range(1, N_DEV):
            cp, nonempty = send_copy(e, d)
            pl.when(nonempty)(cp.wait_send)

    for e in range(E_LOC):
        rows = xg.at[pl.ds(0, 2 * GPAIRS // 8 * 8)]
        pltpu.make_async_copy(rows, rows, xsem.at[e]).wait()
        for _ in range(2 * GPAIRS % 8):
            row1 = xg.at[pl.ds(0, 1)]
            pltpu.make_async_copy(row1, row1, xsem.at[e]).wait()

        xb = xg[pl.ds(e * SLOTS, SLOTS), :].astype(jnp.bfloat16)
        acc = None
        for i, (ce, k0, kb) in enumerate(W_CHUNKS):
            if ce != e:
                continue
            w_copy(i).wait()
            wb = wbuf[e, pl.ds(k0, kb), :].astype(jnp.bfloat16)
            part = jnp.dot(xb[:, k0:k0 + kb], wb, preferred_element_type=jnp.float32)
            acc = part if acc is None else acc + part
        hi = lax.bitcast_convert_type(
            acc[:PAIRS].astype(jnp.bfloat16).astype(jnp.float32), jnp.uint32)
        lo = lax.bitcast_convert_type(
            acc[PAIRS:].astype(jnp.bfloat16).astype(jnp.float32), jnp.uint32)
        packed = hi | (lo >> jnp.uint32(16))
        for g in range(PAIRS // 8):
            for j in range(H // 128):
                sb[pl.ds(e * PAIRS + g * 8, 8), j, :] = (
                    packed[8 * g:8 * g + 8, 128 * j:128 * (j + 1)])
        for d in (2, 1, 3, 0):
            cp, nonempty = send_copy(e, d)
            pl.when(nonempty)(cp.start)
        if e > 0:
            receive(e - 1)
            drain(e - 1)
    receive(E_LOC - 1)
    drain(E_LOC - 1)


def pallas_dist_moe_cap_ep_outshard_n2048_d512_e8_h1024_kernel(x, router_W, route_idx, expert_W):
    del router_W
    idx2d = route_idx.astype(jnp.int32).reshape(NBLK, 128)
    out = pl.pallas_call(
        _body,
        out_shape=jax.ShapeDtypeStruct((TOK_LOC // 8, 8, 8, 128), jnp.float32),
        in_specs=[pl.BlockSpec(memory_space=pltpu.VMEM),
                  pl.BlockSpec(memory_space=pl.ANY),
                  pl.BlockSpec(memory_space=pl.ANY)],
        out_specs=pl.BlockSpec(memory_space=pltpu.VMEM),
        scratch_shapes=[
            pltpu.VMEM((E_LOC, D, H), jnp.float32),
            pltpu.VMEM((E_LOC * SLOTS, D), jnp.float32),
            pltpu.VMEM((E_LOC * PAIRS, 8, 128), jnp.uint32),
            pltpu.VMEM((N_EXP * PAIRS, 8, 128), jnp.uint32),
            pltpu.VMEM((2 * N_EXP, 128), jnp.int32),
            pltpu.SMEM((2 * N_EXP, 128), jnp.int32),
            pltpu.SemaphoreType.DMA((len(W_CHUNKS),)),
            pltpu.SemaphoreType.DMA((E_LOC,)),
            pltpu.SemaphoreType.DMA((E_LOC * N_DEV,)),
            pltpu.SemaphoreType.DMA((N_EXP,)),
            pltpu.SemaphoreType.DMA,
        ],
        compiler_params=pltpu.CompilerParams(
            collective_id=0, vmem_limit_bytes=64 * 1024 * 1024,
            disable_bounds_checks=True, disable_semaphore_checks=True),
    )(idx2d, x, expert_W)
    out = out.transpose(0, 2, 1, 3)
    return out.reshape(TOK_LOC, H)
```

```python
import jax
import jax.numpy as jnp
from jax import lax
from jax.experimental import pallas as pl
from jax.experimental.pallas import tpu as pltpu

N_TOK = 2048
D = 512
H = 1024
N_EXP = 32
N_DEV = 4
E_LOC = N_EXP // N_DEV
CAP = 51
SLOTS = 64
PAIRS = SLOTS // 2
TOK_LOC = N_TOK // N_DEV
NBLK = N_TOK // 128
GPAIRS = (CAP + 1) // 2
KCS = (1, 1, 1, 1, 1, 2, 2, 4)
W_CHUNKS = [(e, kc * (D // n), D // n) for e, n in enumerate(KCS) for kc in range(n)]


def _body(idx_ref, x_hbm, w_hbm, out_ref,
          wbuf, xg, sb, rb, meta_v, meta_s,
          wsem, xsem, ssem, rsem, msem):
    me = lax.axis_index("i")

    def w_copy(i):
        e, k0, kb = W_CHUNKS[i]
        return pltpu.make_async_copy(
            w_hbm.at[e, pl.ds(k0, kb), :], wbuf.at[e, pl.ds(k0, kb), :], wsem.at[i])

    for i in range(len(W_CHUNKS)):
        w_copy(i).start(priority=1)

    barrier = pltpu.get_barrier_semaphore()
    for d in range(1, N_DEV):
        pl.semaphore_signal(barrier, inc=1, device_id=((me + d) % N_DEV,),
                            device_id_type=pl.DeviceIdType.MESH)

    idx = idx_ref[...]
    e_iota = lax.broadcasted_iota(jnp.int32, (NBLK, N_EXP, 128), 1)
    oh_f = jnp.where(idx[:, None, :] == e_iota, 1.0, 0.0).astype(jnp.float32)
    oh2 = oh_f.reshape(NBLK * N_EXP, 128).astype(jnp.bfloat16)
    r_i = lax.broadcasted_iota(jnp.int32, (128, 128), 0)
    c_i = lax.broadcasted_iota(jnp.int32, (128, 128), 1)
    upper = jnp.where(r_i < c_i, 1.0, 0.0).astype(jnp.bfloat16)
    ones = jnp.ones((128, 128), jnp.bfloat16)
    cw = jnp.dot(oh2, upper, preferred_element_type=jnp.float32).reshape(NBLK, N_EXP, 128)
    tot = jnp.dot(oh2, ones, preferred_element_type=jnp.float32).reshape(NBLK, N_EXP, 128)
    carry = jnp.zeros((N_EXP, 128), jnp.float32)
    lane = lax.broadcasted_iota(jnp.int32, (N_EXP, 128), 1)
    bnd = jnp.zeros((N_EXP, 128), jnp.float32)
    slot_iota = lax.broadcasted_iota(jnp.int32, (SLOTS, 128), 0)
    lane_f = lane.astype(jnp.float32)
    a_parts, b_parts = [], []
    for b in range(NBLK):
        if b % (NBLK // N_DEV) == 0:
            bnd = jnp.where(lane == SLOTS + b // (NBLK // N_DEV),
                            jnp.minimum(carry, float(CAP)), bnd)
        cum = cw[b] + carry
        pos = jnp.sum(oh_f[b] * cum, axis=0, keepdims=True)
        pos_i = pos.astype(jnp.int32)
        bt = jnp.where((slot_iota == pos_i) & (slot_iota < CAP), 1.0, 0.0).astype(jnp.bfloat16)
        a_b = jnp.concatenate([oh_f[b] * float(b), oh_f[b] * lane_f],
                              axis=0).astype(jnp.bfloat16)
        a_parts.append(a_b)
        b_parts.append(bt)
        carry = carry + tot[b]
    bnd = jnp.where(lane == SLOTS + N_DEV, jnp.minimum(carry, float(CAP)), bnd)
    a_all = jnp.concatenate(a_parts, axis=1)
    b_all = jnp.concatenate(b_parts, axis=1)
    tk = lax.dot_general(a_all, b_all, (((1,), (1,)), ((), ())),
                         preferred_element_type=jnp.float32)
    tok = tk[:N_EXP] * 128.0 + tk[N_EXP:]
    tok_pad = jnp.concatenate([tok, jnp.zeros((N_EXP, 128 - SLOTS), jnp.float32)], axis=1)
    m0 = jnp.where(lane < SLOTS, tok_pad, bnd).astype(jnp.int32)
    m1 = m0 & (TOK_LOC - 1)
    meta_v[pl.ds(0, N_EXP), :] = m0
    meta_v[pl.ds(N_EXP, N_EXP), :] = m1
    mcp = pltpu.make_async_copy(meta_v, meta_s, msem)
    mcp.start()

    xg[...] = jnp.zeros(xg.shape, xg.dtype)
    out_ref[...] = jnp.zeros(out_ref.shape, out_ref.dtype)
    mcp.wait()

    def x_copies(e, p):
        ge = me * E_LOC + e
        t0 = meta_s[ge, 2 * p]
        t1 = meta_s[ge, 2 * p + 1]
        return (pltpu.make_async_copy(x_hbm.at[pl.ds(t0, 1)],
                                      xg.at[pl.ds(e * SLOTS + p, 1)], xsem.at[e]),
                pltpu.make_async_copy(x_hbm.at[pl.ds(t1, 1)],
                                      xg.at[pl.ds(e * SLOTS + PAIRS + p, 1)], xsem.at[e]))

    for e in range(E_LOC):
        def issue(p, carry_, e=e):
            for cp in x_copies(e, p):
                cp.start()
            return carry_
        lax.fori_loop(0, GPAIRS, issue, 0, unroll=2)

    pl.semaphore_wait(barrier, N_DEV - 1)

    def send_copy(e, d):
        k = (me + d) % N_DEV
        ge = me * E_LOC + e
        s0 = meta_s[ge, SLOTS + k]
        s1 = meta_s[ge, SLOTS + k + 1]
        ps = s0 >> 1
        npair = ((s1 + 1) >> 1) - ps
        src = sb.at[pl.ds(e * PAIRS + ps, npair)]
        dst = rb.at[pl.ds(ge * PAIRS + ps, npair)]
        if d == 0:
            cp = pltpu.make_async_copy(src, dst, rsem.at[ge])
        else:
            cp = pltpu.make_async_remote_copy(
                src_ref=src, dst_ref=dst, send_sem=ssem.at[e * N_DEV + d],
                recv_sem=rsem.at[ge], device_id=(k,),
                device_id_type=pl.DeviceIdType.MESH)
        return cp, s1 > s0

    def receive(e):
        for s in range(N_DEV):
            ge = s * E_LOC + e
            s0 = meta_s[ge, SLOTS + me]
            s1 = meta_s[ge, SLOTS + me + 1]

            @pl.when(s1 > s0)
            def _(ge=ge, s0=s0, s1=s1):
                ps = s0 >> 1
                npair = ((s1 + 1) >> 1) - ps
                dst = rb.at[pl.ds(ge * PAIRS + ps, npair)]
                pltpu.make_async_copy(dst, dst, rsem.at[ge]).wait()

                def place(c, carry_):
                    row = meta_s[N_EXP + ge, c]
                    u = rb[ge * PAIRS + (c >> 1)]
                    sh = ((c & 1) << 4).astype(jnp.uint32)
                    v = lax.bitcast_convert_type(
                        (u << sh) & jnp.uint32(0xFFFF0000), jnp.float32)
                    out_ref[row >> 3, :, row & 7, :] = v
                    return carry_
                lax.fori_loop(s0, s1, place, 0)

    def drain(e):
        for d in range(1, N_DEV):
            cp, nonempty = send_copy(e, d)
            pl.when(nonempty)(cp.wait_send)

    for e in range(E_LOC):
        def xwait(p, carry_, e=e):
            for cp in x_copies(e, p):
                cp.wait()
            return carry_
        lax.fori_loop(0, GPAIRS, xwait, 0)

        xb = xg[pl.ds(e * SLOTS, SLOTS), :].astype(jnp.bfloat16)
        acc = None
        for i, (ce, k0, kb) in enumerate(W_CHUNKS):
            if ce != e:
                continue
            w_copy(i).wait()
            wb = wbuf[e, pl.ds(k0, kb), :].astype(jnp.bfloat16)
            part = jnp.dot(xb[:, k0:k0 + kb], wb, preferred_element_type=jnp.float32)
            acc = part if acc is None else acc + part
        hi = lax.bitcast_convert_type(
            acc[:PAIRS].astype(jnp.bfloat16).astype(jnp.float32), jnp.uint32)
        lo = lax.bitcast_convert_type(
            acc[PAIRS:].astype(jnp.bfloat16).astype(jnp.float32), jnp.uint32)
        packed = hi | (lo >> jnp.uint32(16))
        for g in range(PAIRS // 8):
            for j in range(H // 128):
                sb[pl.ds(e * PAIRS + g * 8, 8), j, :] = (
                    packed[8 * g:8 * g + 8, 128 * j:128 * (j + 1)])
        for d in (2, 1, 3, 0):
            cp, nonempty = send_copy(e, d)
            pl.when(nonempty)(cp.start)
        if e > 0:
            receive(e - 1)
            drain(e - 1)
    receive(E_LOC - 1)
    drain(E_LOC - 1)


def pallas_dist_moe_cap_ep_outshard_n2048_d512_e8_h1024_kernel(x, router_W, route_idx, expert_W):
    del router_W
    idx2d = route_idx.astype(jnp.int32).reshape(NBLK, 128)
    out = pl.pallas_call(
        _body,
        out_shape=jax.ShapeDtypeStruct((TOK_LOC // 8, 8, 8, 128), jnp.float32),
        in_specs=[pl.BlockSpec(memory_space=pltpu.VMEM),
                  pl.BlockSpec(memory_space=pl.ANY),
                  pl.BlockSpec(memory_space=pl.ANY)],
        out_specs=pl.BlockSpec(memory_space=pltpu.VMEM),
        scratch_shapes=[
            pltpu.VMEM((E_LOC, D, H), jnp.float32),
            pltpu.VMEM((E_LOC * SLOTS, D), jnp.float32),
            pltpu.VMEM((E_LOC * PAIRS, 8, 128), jnp.uint32),
            pltpu.VMEM((N_EXP * PAIRS, 8, 128), jnp.uint32),
            pltpu.VMEM((2 * N_EXP, 128), jnp.int32),
            pltpu.SMEM((2 * N_EXP, 128), jnp.int32),
            pltpu.SemaphoreType.DMA((len(W_CHUNKS),)),
            pltpu.SemaphoreType.DMA((E_LOC,)),
            pltpu.SemaphoreType.DMA((E_LOC * N_DEV,)),
            pltpu.SemaphoreType.DMA((N_EXP,)),
            pltpu.SemaphoreType.DMA,
        ],
        compiler_params=pltpu.CompilerParams(
            collective_id=0, vmem_limit_bytes=64 * 1024 * 1024,
            disable_bounds_checks=True, disable_semaphore_checks=True),
    )(idx2d, x, expert_W)
    out = out.transpose(0, 2, 1, 3)
    return out.reshape(TOK_LOC, H)
```
